```python
import numpy as np

kernel_name = "dist_ar_xy_y_m256_n256"

def setup_inputs():
    return {"x": np.random.randn(512, 256).astype(np.float32)}

def reference(x: np.ndarray) -> np.ndarray:
    return x.reshape(2, 256, 256).sum(axis=0)
```

```python
import jax
import jax.numpy as jnp
from jax import lax
from jax.experimental import pallas as pl
from jax.experimental.pallas import tpu as pltpu


def pallas_dist_ar_xy_y_m256_n256_kernel(x: jax.Array):
    m, n = x.shape

    def body(x_ref, out_ref, send_buf, recv_buf, send_sem, recv_sem):
        my_x = lax.axis_index("x")
        my_y = lax.axis_index("y")
        peer = (my_x, 1 - my_y)

        barrier = pltpu.get_barrier_semaphore()
        pl.semaphore_signal(barrier, inc=1, device_id=peer,
                            device_id_type=pl.DeviceIdType.MESH)
        send_buf[...] = x_ref[...].astype(jnp.bfloat16)
        pl.semaphore_wait(barrier, 1)

        rdma = pltpu.make_async_remote_copy(
            src_ref=send_buf, dst_ref=recv_buf,
            send_sem=send_sem, recv_sem=recv_sem,
            device_id=peer, device_id_type=pl.DeviceIdType.MESH)
        rdma.start()
        rdma.wait()
        out_ref[...] = x_ref[...] + recv_buf[...].astype(jnp.float32)

    return pl.pallas_call(
        body,
        out_shape=jax.ShapeDtypeStruct((m, n), jnp.float32),
        in_specs=[pl.BlockSpec(memory_space=pltpu.VMEM)],
        out_specs=pl.BlockSpec(memory_space=pltpu.VMEM),
        scratch_shapes=[
            pltpu.VMEM((m, n), jnp.bfloat16),
            pltpu.VMEM((m, n), jnp.bfloat16),
            pltpu.SemaphoreType.DMA,
            pltpu.SemaphoreType.DMA,
        ],
        compiler_params=pltpu.CompilerParams(collective_id=0),
    )(x)
```

```python
import functools

import jax
import jax.numpy as jnp
from jax import lax
from jax.experimental import pallas as pl
from jax.experimental.pallas import tpu as pltpu

M = 256
N = 256
_MESH = pl.DeviceIdType.MESH
_DEVICES = ((0, 1), (1, 1), (1, 0), (0, 0))


def _tile(h, f32=False):
    return (8 * (h // 2), 8, 128 * (h % 2), 128, f32)


def _cover(h0, h1, counts, f32=False):
    out, h, k = [], h0, 0
    while h < h1:
        n = min(counts[min(k, len(counts) - 1)], h1 - h)
        k += 1
        if h % 2 or n == 1:
            out.append(_tile(h, f32))
            h += 1
        else:
            n -= n % 2
            out.append((4 * h, 4 * n, 0, N, f32))
            h += n
    return out


def _bulk(h0, h1):
    head = [_tile(h0)] if h0 % 2 else []
    h0 += h0 % 2
    return head + _cover(h0, h1 - 4, (16,)) + _cover(h1 - 4, h1, (4,))


def _schedule():
    tiles = M // 4
    fwd_to_00 = 12
    head_11 = 1
    head_01 = 3
    fwd = 12
    p0 = tiles - fwd

    y_send, n_fwd, loads = {}, {}, {}
    first = (_cover(fwd_to_00 - head_11, fwd_to_00, (1,), True)
             + _cover(0, fwd_to_00 - head_11, (1,)))
    y_send[(1, 1)] = first + _bulk(fwd_to_00, p0)
    n_fwd[(1, 0)] = range(len(first))
    head = _cover(fwd_to_00, fwd_to_00 + head_01, (2,), True)
    first = _cover(p0, tiles, (1, 1, 2, 4))
    y_send[(0, 1)] = head + first + _bulk(fwd_to_00 + head_01, p0)
    n_fwd[(0, 0)] = range(len(head), len(head) + len(first))
    for x in range(2):
        first = _cover(x * fwd, (x + 1) * fwd, (4,))
        y_send[(x, 0)] = first + _bulk(2 * fwd, tiles)
        n_fwd[(x, 1)] = range(len(first))
    lo = _cover(0, 20, (1, 1, 2, 4, 12))
    hi = _cover(p0, tiles, (1, 1, 2, 8))
    mid = _cover(20, p0, (tiles,))
    loads[(1, 1)] = lo + mid + _cover(p0, tiles, (tiles,))
    loads[(0, 1)] = hi + _cover(0, p0, (tiles,))
    loads[(0, 0)] = loads[(1, 0)] = _cover(0, tiles, (tiles,))
    return y_send, n_fwd, loads


_Y_SEND, _FWD, _LOADS = _schedule()
_EARLY_LOADS_11 = 4


def _view(ref, p):
    if p[3] == N:
        return ref.at[pl.ds(p[0], p[1])]
    return ref.at[pl.ds(p[0], p[1]), pl.ds(p[2], p[3])]


def _idx(p):
    return (pl.ds(p[0], p[1]), pl.ds(p[2], p[3]))


def _overlap(p, q):
    return (p[0] < q[0] + q[1] and q[0] < p[0] + p[1]
            and p[2] < q[2] + q[3] and q[2] < p[2] + p[3])


def _body(x_hbm, out, x_vmem, send16, recv16, recv32,
          load_sems, y_send_sems, y_recv_sems, x_send_sems, x_recv_sems, ready):
    my_x = lax.axis_index("x")
    my_y = lax.axis_index("y")
    barrier = pltpu.get_barrier_semaphore()

    @pl.when(my_x != my_y)
    def _():
        for d in ((1, 1), (0, 0)):
            pl.semaphore_signal(barrier, inc=1, device_id=d, device_id_type=_MESH)

    def program(me):
        y_peer = (me[0], 1 - me[1])
        x_peer = (1 - me[0], me[1])
        diag = (1 - me[0], 1 - me[1])
        y_out, y_in = _Y_SEND[me], _Y_SEND[y_peer]
        x_in = [_Y_SEND[diag][i] for i in _FWD[x_peer]]

        def recv_buf(p):
            return recv32 if p[4] else recv16

        def remote(src, p, send_sem, recv_sem, peer):
            return pltpu.make_async_remote_copy(
                src_ref=_view(src, p), dst_ref=_view(recv_buf(p), p),
                send_sem=send_sem, recv_sem=recv_sem,
                device_id=peer, device_id_type=_MESH)

        loads = [pltpu.make_async_copy(_view(x_hbm, p), _view(x_vmem, p),
                                       load_sems.at[i])
                 for i, p in enumerate(_LOADS[me])]
        pending = set(range(len(loads)))

        def wait_loaded(p):
            for i in sorted(pending):
                if _overlap(p, _LOADS[me][i]):
                    loads[i].wait()
                    pending.discard(i)

        def convert(p):
            wait_loaded(p)
            send16[_idx(p)] = x_vmem[_idx(p)].astype(jnp.bfloat16)

        def add(p):
            out[_idx(p)] = x_vmem[_idx(p)] + recv_buf(p)[_idx(p)].astype(jnp.float32)

        y_sends = [remote(x_hbm if p[4] else send16, p, y_send_sems.at[i],
                          y_recv_sems.at[i], y_peer)
                   for i, p in enumerate(y_out)]
        n_head = sum(p[4] for p in y_out)
        everything = (0, M, 0, N)

        if me == (0, 1):
            loads[0].start()
            pl.semaphore_wait(barrier, 1)
            for c in y_sends[:n_head] + loads[1:]:
                c.start()
            for p, c in list(zip(y_out, y_sends))[n_head:]:
                convert(p)
                c.start()
            wait_loaded(everything)
            pl.semaphore_wait(ready, 1)
        elif me == (1, 1):
            for c in loads[:_EARLY_LOADS_11]:
                c.start()
            pl.semaphore_wait(barrier, 2)
            for c in y_sends[:n_head] + loads[_EARLY_LOADS_11:]:
                c.start()
            for d in (y_peer, x_peer):
                pl.semaphore_signal(ready, inc=1, device_id=d, device_id_type=_MESH)
            for p, c in list(zip(y_out, y_sends))[n_head:]:
                convert(p)
                c.start()
            wait_loaded(everything)
        else:
            if me == (0, 0):
                for d in (y_peer, x_peer):
                    pl.semaphore_signal(barrier, inc=1, device_id=d,
                                        device_id_type=_MESH)
            for c in loads:
                c.start()
            for p in y_out:
                convert(p)
            if me == (0, 0):
                pl.semaphore_wait(barrier, 2)
            else:
                pl.semaphore_wait(barrier, 1)
                pl.semaphore_wait(ready, 1)
            for c in y_sends:
                c.start()

        y_recvs = [remote(recv_buf(p), p, y_send_sems.at[i], y_recv_sems.at[i],
                          y_peer)
                   for i, p in enumerate(y_in)]
        x_recvs = [remote(recv_buf(p), p, x_send_sems.at[j], x_recv_sems.at[j],
                          x_peer)
                   for j, p in enumerate(x_in)]
        x_sends = {i: remote(recv_buf(y_in[i]), y_in[i], x_send_sems.at[j],
                             x_recv_sems.at[j], x_peer)
                   for j, i in enumerate(_FWD[me])}

        deferred = []
        for i, p in enumerate(y_in[:-1]):
            y_recvs[i].wait_recv()
            deferred.append(p)
            if i in x_sends:
                x_sends[i].start()
            if i + 1 not in x_sends:
                for q in deferred:
                    add(q)
                deferred = []
        for c in y_sends + list(x_sends.values()):
            c.wait_send()
        for c, p in list(zip(x_recvs, x_in))[:-1]:
            c.wait_recv()
            add(p)
        y_recvs[-1].wait_recv()
        add(y_in[-1])
        x_recvs[-1].wait_recv()
        add(x_in[-1])

    for d in _DEVICES:
        pl.when(jnp.logical_and(my_x == d[0], my_y == d[1]))(
            functools.partial(program, d))


def _compiler_params():
    try:
        return pltpu.CompilerParams(collective_id=0, disable_bounds_checks=True,
                                    disable_semaphore_checks=True)
    except TypeError:
        return pltpu.CompilerParams(collective_id=0)


def pallas_dist_ar_xy_y_m256_n256_kernel(x: jax.Array):
    assert x.shape == (M, N), x.shape
    n_load = max(len(v) for v in _LOADS.values())
    n_y = max(len(v) for v in _Y_SEND.values())
    n_x = max(len(v) for v in _FWD.values())
    return pl.pallas_call(
        _body,
        out_shape=jax.ShapeDtypeStruct((M, N), jnp.float32),
        in_specs=[pl.BlockSpec(memory_space=pl.ANY)],
        out_specs=pl.BlockSpec(memory_space=pltpu.VMEM),
        scratch_shapes=[
            pltpu.VMEM((M, N), jnp.float32),
            pltpu.VMEM((M, N), jnp.bfloat16),
            pltpu.VMEM((M, N), jnp.bfloat16),
            pltpu.VMEM((M, N), jnp.float32),
            pltpu.SemaphoreType.DMA((n_load,)),
            pltpu.SemaphoreType.DMA((n_y,)),
            pltpu.SemaphoreType.DMA((n_y,)),
            pltpu.SemaphoreType.DMA((n_x,)),
            pltpu.SemaphoreType.DMA((n_x,)),
            pltpu.SemaphoreType.REGULAR,
        ],
        compiler_params=_compiler_params(),
    )(x)
```

```python
import functools

import jax
import jax.numpy as jnp
from jax import lax
from jax.experimental import pallas as pl
from jax.experimental.pallas import tpu as pltpu

M = 256
N = 256
_MESH = pl.DeviceIdType.MESH
_DEVICES = ((0, 1), (1, 1), (1, 0), (0, 0))
_TILES = (M // 8) * (N // 128)


def _tile(h, f32=False):
    return (8 * (h // 2), 8, 128 * (h % 2), 128, f32)


def _cover(h0, h1, counts, f32=False):
    out, h, k = [], h0, 0
    while h < h1:
        n = min(counts[min(k, len(counts) - 1)], h1 - h)
        k += 1
        if h % 2 or n == 1:
            out.append(_tile(h, f32))
            h += 1
        else:
            n -= n % 2
            out.append((4 * h, 4 * n, 0, N, f32))
            h += n
    return out


def _bulk(h0, h1):
    head = [_tile(h0)] if h0 % 2 else []
    h0 += h0 % 2
    return head + _cover(h0, h1 - 4, (16,)) + _cover(h1 - 4, h1, (4,))


def _stripes(p):
    return [[2 * r + c for c in range(p[2] // 128, (p[2] + p[3]) // 128)]
            for r in range(p[0] // 8, (p[0] + p[1]) // 8)]


def _schedule():
    fwd_to_00 = 12
    head_11 = 1
    head_01 = 3
    fwd = 12
    p0 = _TILES - fwd

    y_send, fwd_idx, early = {}, {}, {}
    first = (_cover(fwd_to_00 - head_11, fwd_to_00, (1,), True)
             + _cover(0, fwd_to_00 - head_11, (1,)))
    y_send[(1, 1)] = first + _bulk(fwd_to_00, p0)
    fwd_idx[(1, 0)] = range(len(first))
    head = _cover(fwd_to_00, fwd_to_00 + head_01, (1,), True)
    first = _cover(p0, _TILES, (1, 1, 2, 2, 2, 4))
    y_send[(0, 1)] = head + first + _bulk(fwd_to_00 + head_01, p0)
    fwd_idx[(0, 0)] = range(len(head), len(head) + len(first))
    for x in range(2):
        first = _cover(x * fwd, (x + 1) * fwd, (4,))
        y_send[(x, 0)] = first + _bulk(2 * fwd, _TILES)
        fwd_idx[(x, 1)] = range(len(first))
    early[(1, 1)] = list(range(fwd_to_00 - head_11))
    early[(0, 1)] = list(range(p0, _TILES))
    early[(0, 0)] = early[(1, 0)] = []

    urgent = {12: 0, 13: 5, 14: 9, 11: 12,
              0: 17, 1: 20, 2: 23, 3: 30, 4: 31, 5: 38,
              6: 60, 7: 57, 8: 54, 9: 47, 10: 46,
              52: 40, 53: 45, 54: 48, 55: 53, 56: 58, 57: 59,
              58: 39, 59: 37, 60: 32, 61: 29, 62: 24, 63: 19}
    rest = iter(h for h in range(_TILES) if h not in urgent.values())
    perm = [urgent[s] if s in urgent else next(rest) for s in range(_TILES)]
    assert sorted(perm) == list(range(_TILES))
    return y_send, fwd_idx, early, perm


_Y_SEND, _FWD, _EARLY, _PERM_B = _schedule()
_ROW_LOADS = {0: ((0, M),), 1: ((0, 96), (96, M - 96))}


def _idx(p):
    return (pl.ds(p[0], p[1]), pl.ds(p[2], p[3]))


def _view(ref, p):
    if p[3] == N:
        return ref.at[pl.ds(p[0], p[1])]
    return ref.at[_idx(p)]


def _body(x_hbm, out, x_vmem, stage, send16, recv16, recv32,
          load_sems, y_send_sems, y_recv_sems, x_send_sems, x_recv_sems, ready):
    my_x = lax.axis_index("x")
    my_y = lax.axis_index("y")
    barrier = pltpu.get_barrier_semaphore()

    @pl.when(my_x != my_y)
    def _():
        for d in ((1, 1), (0, 0)):
            pl.semaphore_signal(barrier, inc=1, device_id=d, device_id_type=_MESH)

    def program(me):
        y_peer = (me[0], 1 - me[1])
        x_peer = (1 - me[0], me[1])
        diag = (1 - me[0], 1 - me[1])
        holds_b = me[1] == 1
        y_out, y_in = _Y_SEND[me], _Y_SEND[y_peer]
        x_in = [_Y_SEND[diag][i] for i in _FWD[x_peer]]
        early, row_loads = _EARLY[me], _ROW_LOADS[me[1]]

        def recv_buf(p):
            return recv32 if p[4] else recv16

        def remote(src, p, send_sem, recv_sem, peer):
            return pltpu.make_async_remote_copy(
                src_ref=src, dst_ref=_view(recv_buf(p), p),
                send_sem=send_sem, recv_sem=recv_sem,
                device_id=peer, device_id_type=_MESH)

        loads = [pltpu.make_async_copy(_view(x_hbm, _tile(_PERM_B[s])),
                                       _view(stage, _tile(s)), load_sems.at[i])
                 for i, s in enumerate(early)]
        loads += [pltpu.make_async_copy(x_hbm.at[pl.ds(r0, rows)],
                                        x_vmem.at[pl.ds(r0, rows)],
                                        load_sems.at[len(early) + i])
                  for i, (r0, rows) in enumerate(row_loads)]
        pending = set(range(len(loads)))

        def wait_load(i):
            if i in pending:
                loads[i].wait()
                pending.discard(i)

        def wait_all_loads():
            for i in sorted(pending):
                wait_load(i)

        def b_slot(s):
            if s in early:
                wait_load(early.index(s))
                return stage[_idx(_tile(s))]
            t = _tile(_PERM_B[s])
            for i, (r0, rows) in enumerate(row_loads):
                if r0 <= t[0] < r0 + rows:
                    wait_load(len(early) + i)
            return x_vmem[_idx(t)]

        def convert(p):
            if not holds_b:
                wait_all_loads()
                send16[_idx(p)] = x_vmem[_idx(p)].astype(jnp.bfloat16)
                return
            for slots in _stripes(p):
                v = [b_slot(s) for s in slots]
                v = v[0] if len(v) == 1 else jnp.concatenate(v, axis=1)
                send16[pl.ds(8 * (slots[0] // 2), 8), pl.ds(p[2], p[3])] = (
                    v.astype(jnp.bfloat16))

        def add(p):
            buf = recv_buf(p)
            if holds_b:
                out[_idx(p)] = x_vmem[_idx(p)] + buf[_idx(p)].astype(jnp.float32)
                return
            for slots in _stripes(p):
                v = buf[pl.ds(8 * (slots[0] // 2), 8), pl.ds(p[2], p[3])]
                v = v.astype(jnp.float32)
                for k, s in enumerate(slots):
                    t = _idx(_tile(_PERM_B[s]))
                    out[t] = x_vmem[t] + v[:, 128 * k:128 * (k + 1)]

        def y_source(p):
            if p[4]:
                (s,), = _stripes(p)
                return _view(x_hbm, _tile(_PERM_B[s]))
            return _view(send16, p)

        y_sends = [remote(y_source(p), p, y_send_sems.at[i], y_recv_sems.at[i],
                          y_peer)
                   for i, p in enumerate(y_out)]
        n_head = sum(p[4] for p in y_out)

        if me == (0, 1):
            loads[0].start()
            pl.semaphore_wait(barrier, 1)
            for c in y_sends[:n_head] + loads[1:]:
                c.start()
            for p, c in list(zip(y_out, y_sends))[n_head:]:
                convert(p)
                c.start()
            wait_all_loads()
            pl.semaphore_wait(ready, 1)
        elif me == (1, 1):
            for c in loads[:len(early)]:
                c.start()
            pl.semaphore_wait(barrier, 2)
            for c in y_sends[:n_head] + loads[len(early):]:
                c.start()
            for d in (y_peer, x_peer):
                pl.semaphore_signal(ready, inc=1, device_id=d, device_id_type=_MESH)
            for p, c in list(zip(y_out, y_sends))[n_head:]:
                convert(p)
                c.start()
            wait_all_loads()
        else:
            if me == (0, 0):
                for d in (y_peer, x_peer):
                    pl.semaphore_signal(barrier, inc=1, device_id=d,
                                        device_id_type=_MESH)
            for c in loads:
                c.start()
            for p in y_out:
                convert(p)
            if me == (0, 0):
                pl.semaphore_wait(barrier, 2)
            else:
                pl.semaphore_wait(barrier, 1)
                pl.semaphore_wait(ready, 1)
            for c in y_sends:
                c.start()

        def in_place(p, send_sem, recv_sem, peer):
            return remote(_view(recv_buf(p), p), p, send_sem, recv_sem, peer)

        y_recvs = [in_place(p, y_send_sems.at[i], y_recv_sems.at[i], y_peer)
                   for i, p in enumerate(y_in)]
        x_recvs = [in_place(p, x_send_sems.at[j], x_recv_sems.at[j], x_peer)
                   for j, p in enumerate(x_in)]
        x_sends = {i: in_place(y_in[i], x_send_sems.at[j], x_recv_sems.at[j],
                               x_peer)
                   for j, i in enumerate(_FWD[me])}

        n, m = len(y_in), len(x_in)
        y_late, x_split = (2, m - 5) if me == (0, 0) else (1, m - 1)
        tail = [(x_recvs[j], x_in[j]) for j in range(x_split)]
        tail += [(y_recvs[i], y_in[i]) for i in range(n - y_late, n - 1)]
        tail += [(x_recvs[j], x_in[j]) for j in range(x_split, m - 1)]
        tail += [(y_recvs[-1], y_in[-1]), (x_recvs[-1], x_in[-1])]

        deferred = []
        for i, p in enumerate(y_in[:n - y_late]):
            y_recvs[i].wait_recv()
            deferred.append(p)
            if i in x_sends:
                x_sends[i].start()
            if i not in x_sends or i + 1 not in x_sends:
                for q in deferred:
                    add(q)
                deferred = []
        for c in y_sends + list(x_sends.values()):
            c.wait_send()
        for c, p in tail:
            c.wait_recv()
            add(p)

    for d in _DEVICES:
        pl.when(jnp.logical_and(my_x == d[0], my_y == d[1]))(
            functools.partial(program, d))


def _compiler_params():
    try:
        return pltpu.CompilerParams(collective_id=0, disable_bounds_checks=True,
                                    disable_semaphore_checks=True)
    except TypeError:
        return pltpu.CompilerParams(collective_id=0)


def pallas_dist_ar_xy_y_m256_n256_kernel(x: jax.Array):
    assert x.shape == (M, N), x.shape
    n_load = max(len(_EARLY[d]) + len(_ROW_LOADS[d[1]]) for d in _DEVICES)
    n_y = max(len(v) for v in _Y_SEND.values())
    n_x = max(len(v) for v in _FWD.values())
    return pl.pallas_call(
        _body,
        out_shape=jax.ShapeDtypeStruct((M, N), jnp.float32),
        in_specs=[pl.BlockSpec(memory_space=pl.ANY)],
        out_specs=pl.BlockSpec(memory_space=pltpu.VMEM),
        scratch_shapes=[
            pltpu.VMEM((M, N), jnp.float32),
            pltpu.VMEM((M, N), jnp.float32),
            pltpu.VMEM((M, N), jnp.bfloat16),
            pltpu.VMEM((M, N), jnp.bfloat16),
            pltpu.VMEM((M, N), jnp.float32),
            pltpu.SemaphoreType.DMA((n_load,)),
            pltpu.SemaphoreType.DMA((n_y,)),
            pltpu.SemaphoreType.DMA((n_y,)),
            pltpu.SemaphoreType.DMA((n_x,)),
            pltpu.SemaphoreType.DMA((n_x,)),
            pltpu.SemaphoreType.REGULAR,
        ],
        compiler_params=_compiler_params(),
    )(x)
```

```python
import functools

import jax
import jax.numpy as jnp
from jax import lax
from jax.experimental import pallas as pl
from jax.experimental.pallas import tpu as pltpu

M = 256
N = 256
_MESH = pl.DeviceIdType.MESH
_DEVICES = ((0, 1), (1, 1), (1, 0), (0, 0))

_TILES = 64
_ROWS = 8 * _TILES

_URGENT_01 = ((2, 1), (59, 0), (42, 1), (12, 1), (36, 0), (5, 0), (14, 0), (23, 1),
              (15, 0), (38, 1), (50, 1), (31, 1), (7, 0), (48, 0), (43, 1), (53, 0),
              (51, 1), (17, 1), (0, 1), (9, 0), (17, 0), (23, 0), (31, 0), (40, 1),
              (48, 1), (58, 1), (2, 0), (7, 1), (15, 1), (25, 1))
_URGENT_11 = ((33, 0), (9, 1), (3, 1), (40, 0), (28, 0), (58, 0), (25, 0), (0, 0),
              (56, 1), (30, 1), (22, 0), (20, 1), (61, 1), (45, 0), (5, 1), (12, 0),
              (20, 0), (30, 0), (38, 0), (45, 1), (53, 1), (59, 1), (3, 0), (14, 1),
              (22, 1))
_HEAD_01 = 6
_HEAD_11 = 3
_FWD_A = 12
_LOADS_BEFORE_BARRIER = {(0, 1): 2, (1, 1): 16}


def _split(kind, lo, hi, counts):
    out = []
    while lo < hi:
        n = min(counts[min(len(out), len(counts) - 1)], hi - lo)
        out.append((kind, lo, n))
        lo += n
    return out


def _schedule():
    cut = sorted({t for t, _ in _URGENT_01 + _URGENT_11})
    whole = [t for t in range(_TILES) if t not in cut]
    rest = [(t, p) for t in cut for p in range(2)
            if (t, p) not in _URGENT_01 + _URGENT_11]
    halves = (list(_URGENT_11) + list(_URGENT_01[:_HEAD_01]) + rest
              + list(_URGENT_01[_HEAD_01:]))
    assert len(set(halves)) == 2 * len(cut) and len(whole) % 2 == 0
    u1 = 2 * len(_URGENT_11)
    u2 = u1 + 2 * _HEAD_01
    u3 = u2 + 2 * len(rest)
    u4 = 2 * len(halves)

    def bulk(lo, hi, extra=()):
        tiles = _split("t", lo, hi - 2, (16,)) + [("t", hi - 2, 2)]
        return tiles[:1] + list(extra) + tiles[1:]

    y_send, fwd = {}, {}
    first = _split("f", 0, 2 * _HEAD_11, (1,)) + _split("u", 2 * _HEAD_11, u1, (1,))
    y_send[(1, 1)] = first + bulk(0, len(whole), [("u", u1, u3 - u1)])
    fwd[(1, 0)] = range(len(first))
    head = _split("f", u1, u2, (2,))
    first = _split("u", u3, u4, (2, 2, 4, 4, 4, 8))
    y_send[(0, 1)] = head + first + bulk(0, len(whole), [("u", u2, u3 - u2)])
    fwd[(0, 0)] = range(len(head), len(head) + len(first))
    for x in range(2):
        first = _split("t", x * _FWD_A, (x + 1) * _FWD_A, (4,))
        y_send[(x, 0)] = first + bulk(2 * _FWD_A, _TILES)
        fwd[(x, 1)] = range(len(first))

    early = {(1, 1): list(range(_HEAD_11, u1 // 2)),
             (0, 1): list(range(u3 // 2, u4 // 2)), (0, 0): [], (1, 0): []}
    cut_row = 8 * (whole[15] + 1)
    row_loads = {0: ((0, _ROWS),), 1: ((0, cut_row), (cut_row, _ROWS - cut_row))}
    return whole, halves, y_send, fwd, early, row_loads


_WHOLE, _HALVES, _Y_SEND, _FWD, _EARLY, _ROW_LOADS = _schedule()


def _tile_rows(t, n=1):
    return pl.ds(8 * t, 8 * n)


def _unit_rows(u):
    t, parity = _HALVES[u // 2]
    return pl.ds(8 * t + 4 * (u % 2) + parity, 2, stride=2)


def _body(x_tiles, x_units, out, x_vmem, stage, send_t, recv_t, send_u, recv_u,
          recv_f, load_sems, y_send_sems, y_recv_sems, x_send_sems, x_recv_sems,
          ready):
    my_x = lax.axis_index("x")
    my_y = lax.axis_index("y")
    barrier = pltpu.get_barrier_semaphore()

    def signal(sem, dev):
        pl.semaphore_signal(sem, inc=1, device_id=dev, device_id_type=_MESH)

    @pl.when(my_x == 1)
    def _():
        signal(barrier, (1, 1 - my_y))

    def program(me):
        y_peer = (me[0], 1 - me[1])
        x_peer = (1 - me[0], me[1])
        diag = (1 - me[0], 1 - me[1])
        holds_b = me[1] == 1
        y_out, y_in = _Y_SEND[me], _Y_SEND[y_peer]
        x_in = [_Y_SEND[diag][i] for i in _FWD[x_peer]]
        early, row_loads = _EARLY[me], _ROW_LOADS[me[1]]

        def hbm_units(u, n):
            t, parity = _HALVES[u // 2]
            return x_units.at[t, pl.ds(u % 2, n), :, parity, 0, :]

        def recv_view(p):
            kind, lo, n = p
            if kind == "t":
                return recv_t.at[_tile_rows(lo, n)]
            return (recv_u if kind == "u" else recv_f).at[pl.ds(lo, n)]

        def send_view(p):
            kind, lo, n = p
            if kind == "t":
                return send_t.at[_tile_rows(lo, n)]
            return send_u.at[pl.ds(lo, n)] if kind == "u" else hbm_units(lo, n)

        def remote(src, p, send_sem, recv_sem, peer):
            return pltpu.make_async_remote_copy(
                src_ref=src, dst_ref=recv_view(p), send_sem=send_sem,
                recv_sem=recv_sem, device_id=peer, device_id_type=_MESH)

        loads = [pltpu.make_async_copy(hbm_units(2 * h, 2),
                                       stage.at[pl.ds(2 * i, 2)], load_sems.at[i])
                 for i, h in enumerate(early)]
        loads += [pltpu.make_async_copy(x_tiles.at[pl.ds(r0, rows)],
                                        x_vmem.at[pl.ds(r0, rows)],
                                        load_sems.at[len(early) + i])
                  for i, (r0, rows) in enumerate(row_loads)]
        pending = set(range(len(loads)))

        def wait_load(i):
            if i in pending:
                loads[i].wait()
                pending.discard(i)

        def wait_tile(t):
            for i, (r0, rows) in enumerate(row_loads):
                if r0 <= 8 * t < r0 + rows:
                    wait_load(len(early) + i)

        converted = set()

        def convert(p):
            kind, lo, n = p
            if kind == "u":
                for h in range(lo // 2, (lo + n + 1) // 2):
                    if h in converted:
                        continue
                    converted.add(h)
                    for u in (2 * h, 2 * h + 1):
                        if h in early:
                            wait_load(early.index(h))
                            v = stage[2 * early.index(h) + u % 2]
                        else:
                            wait_tile(_HALVES[h][0])
                            v = x_vmem[_unit_rows(u), :]
                        send_u[u] = v.astype(jnp.bfloat16)
            elif not holds_b:
                wait_tile(0)
                rows = _tile_rows(lo, n)
                send_t[rows, :] = x_vmem[rows, :].astype(jnp.bfloat16)
            else:
                for s in range(lo, lo + n, 2):
                    for t in _WHOLE[s:s + 2]:
                        wait_tile(t)
                    v = jnp.concatenate(
                        [x_vmem[_tile_rows(t), :] for t in _WHOLE[s:s + 2]], axis=0)
                    send_t[_tile_rows(s, 2), :] = v.astype(jnp.bfloat16)

        def add(p):
            kind, lo, n = p
            if kind != "t":
                buf = recv_u if kind == "u" else recv_f
                for u in range(lo, lo + n):
                    rows = _unit_rows(u)
                    out[rows, :] = x_vmem[rows, :] + buf[u].astype(jnp.float32)
            elif holds_b:
                rows = _tile_rows(lo, n)
                out[rows, :] = x_vmem[rows, :] + recv_t[rows, :].astype(jnp.float32)
            else:
                for s in range(lo, lo + n, 2):
                    v = recv_t[_tile_rows(s, 2), :].astype(jnp.float32)
                    for j, t in enumerate(_WHOLE[s:s + 2]):
                        rows = _tile_rows(t)
                        out[rows, :] = x_vmem[rows, :] + v[8 * j:8 * j + 8]

        y_sends = [remote(send_view(p), p, y_send_sems.at[i], y_recv_sems.at[i],
                          y_peer)
                   for i, p in enumerate(y_out)]

        if holds_b:
            n_head = sum(p[0] == "f" for p in y_out)
            n_first = _LOADS_BEFORE_BARRIER[me]
            for c in loads[:n_first]:
                c.start()
            pl.semaphore_wait(barrier, 1)
            for c in y_sends[:n_head]:
                c.start()
            if me == (0, 1):
                signal(barrier, y_peer)
            for c in loads[n_first:]:
                c.start()
            for p, c in list(zip(y_out, y_sends))[n_head:]:
                convert(p)
                c.start()
            for i in sorted(pending):
                wait_load(i)
            pl.semaphore_wait(ready, 1)
        else:
            signal(barrier, (0, 1) if me == (0, 0) else (0, 0))
            for c in loads:
                c.start()
            for p in y_out:
                convert(p)
            pl.semaphore_wait(barrier, 2)
            if me == (0, 0):
                signal(barrier, x_peer)
            for c in y_sends:
                c.start()
            if me == (1, 0):
                signal(ready, diag)
                signal(ready, y_peer)

        y_recvs = [remote(recv_view(p), p, y_send_sems.at[i], y_recv_sems.at[i],
                          y_peer)
                   for i, p in enumerate(y_in)]
        x_recvs = [remote(recv_view(p), p, x_send_sems.at[j], x_recv_sems.at[j],
                          x_peer)
                   for j, p in enumerate(x_in)]
        x_sends = {i: remote(recv_view(y_in[i]), y_in[i], x_send_sems.at[j],
                             x_recv_sems.at[j], x_peer)
                   for j, i in enumerate(_FWD[me])}

        n, m = len(y_in), len(x_in)
        y_late, x_split = (2, m - 6) if me == (0, 0) else (1, m - 1)
        deferred = []
        for i, p in enumerate(y_in[:n - y_late]):
            y_recvs[i].wait_recv()
            deferred.append(p)
            if i in x_sends:
                x_sends[i].start()
            if i not in x_sends or i + 1 not in x_sends:
                for q in deferred:
                    add(q)
                deferred = []
        for c in y_sends + list(x_sends.values()):
            c.wait_send()
        tail = [(x_recvs[j], x_in[j]) for j in range(x_split)]
        tail += [(y_recvs[i], y_in[i]) for i in range(n - y_late, n - 1)]
        tail += [(x_recvs[j], x_in[j]) for j in range(x_split, m - 1)]
        for c, p in tail:
            c.wait_recv()
            add(p)
        y_recvs[-1].wait_recv()
        x_recvs[-1].wait_recv()
        add(y_in[-1])
        add(x_in[-1])

    for d in _DEVICES:
        pl.when(jnp.logical_and(my_x == d[0], my_y == d[1]))(
            functools.partial(program, d))


def _compiler_params():
    try:
        return pltpu.CompilerParams(collective_id=0, disable_bounds_checks=True,
                                    disable_semaphore_checks=True)
    except TypeError:
        return pltpu.CompilerParams(collective_id=0)


def pallas_dist_ar_xy_y_m256_n256_kernel(x: jax.Array):
    assert x.shape == (M, N), x.shape
    n_early = max(len(v) for v in _EARLY.values())
    n_load = max(len(_EARLY[d]) + len(_ROW_LOADS[d[1]]) for d in _DEVICES)
    n_y = max(len(v) for v in _Y_SEND.values())
    n_x = max(len(v) for v in _FWD.values())
    n_units = 2 * len(_HALVES)
    tiles = x.reshape(M // 8, 8, N // 128, 128).transpose(0, 2, 1, 3)
    out = pl.pallas_call(
        _body,
        out_shape=jax.ShapeDtypeStruct((_ROWS, 128), jnp.float32),
        in_specs=[pl.BlockSpec(memory_space=pl.ANY)] * 2,
        out_specs=pl.BlockSpec(memory_space=pltpu.VMEM),
        scratch_shapes=[
            pltpu.VMEM((_ROWS, 128), jnp.float32),
            pltpu.VMEM((2 * n_early, 2, 128), jnp.float32),
            pltpu.VMEM((_ROWS, 128), jnp.bfloat16),
            pltpu.VMEM((_ROWS, 128), jnp.bfloat16),
            pltpu.VMEM((n_units, 2, 128), jnp.bfloat16),
            pltpu.VMEM((n_units, 2, 128), jnp.bfloat16),
            pltpu.VMEM((n_units, 2, 128), jnp.float32),
            pltpu.SemaphoreType.DMA((n_load,)),
            pltpu.SemaphoreType.DMA((n_y,)),
            pltpu.SemaphoreType.DMA((n_y,)),
            pltpu.SemaphoreType.DMA((n_x,)),
            pltpu.SemaphoreType.DMA((n_x,)),
            pltpu.SemaphoreType.REGULAR,
        ],
        compiler_params=_compiler_params(),
    )(tiles.reshape(_ROWS, 128), tiles.reshape(_TILES, 2, 2, 2, 1, 128))
    return out.reshape(M // 8, N // 128, 8, 128).transpose(0, 2, 1, 3).reshape(M, N)
```

```python
import functools

import jax
import jax.numpy as jnp
from jax import lax
from jax.experimental import pallas as pl
from jax.experimental.pallas import tpu as pltpu

M = 256
N = 256
_MESH = pl.DeviceIdType.MESH
_DEVICES = ((0, 1), (1, 1), (1, 0), (0, 0))

_TILES = 64
_ROWS = 8 * _TILES

_URGENT_01 = ((2, 1), (59, 0), (42, 1), (12, 1), (36, 0), (5, 0), (14, 0), (23, 1),
              (15, 0), (38, 1), (50, 1), (31, 1), (7, 0), (48, 0), (43, 1), (53, 0),
              (51, 1), (17, 1), (0, 1), (9, 0), (17, 0), (23, 0), (31, 0), (40, 1),
              (48, 1), (58, 1), (2, 0), (7, 1), (15, 1), (25, 1))
_URGENT_11 = ((33, 0), (9, 1), (3, 1), (40, 0), (28, 0), (58, 0), (25, 0), (0, 0),
              (56, 1), (30, 1), (22, 0), (20, 1), (61, 1), (45, 0), (5, 1), (12, 0),
              (20, 0), (30, 0), (38, 0), (45, 1), (53, 1), (59, 1), (3, 0), (14, 1),
              (22, 1))
_HEAD_01 = 6
_HEAD_11 = 3
_FWD_A = 12
_LOADS_BEFORE_BARRIER = {(0, 1): 1, (1, 1): 16}


def _split(kind, lo, hi, counts):
    out = []
    while lo < hi:
        n = min(counts[min(len(out), len(counts) - 1)], hi - lo)
        out.append((kind, lo, n))
        lo += n
    return out


def _schedule():
    cut = sorted({t for t, _ in _URGENT_01 + _URGENT_11})
    whole = [t for t in range(_TILES) if t not in cut]
    rest = [(t, p) for t in cut for p in range(2)
            if (t, p) not in _URGENT_01 + _URGENT_11]
    halves = (list(_URGENT_11) + list(_URGENT_01[:_HEAD_01]) + rest
              + list(_URGENT_01[_HEAD_01:]))
    assert len(set(halves)) == 2 * len(cut) and len(whole) % 2 == 0
    u1 = 2 * len(_URGENT_11)
    u2 = u1 + 2 * _HEAD_01
    u3 = u2 + 2 * len(rest)
    u4 = 2 * len(halves)

    def bulk(lo, hi, extra=()):
        tiles = _split("t", lo, hi - 2, (8, 16)) + [("t", hi - 2, 2)]
        return tiles[:2] + list(extra) + tiles[2:]

    y_send, fwd = {}, {}
    first = _split("f", 0, 2 * _HEAD_11, (1,)) + _split("u", 2 * _HEAD_11, u1, (1,))
    y_send[(1, 1)] = first + bulk(0, len(whole), [("u", u1, u3 - u1)])
    fwd[(1, 0)] = range(len(first))
    head = _split("f", u1, u2, (2,))
    first = _split("u", u3, u4, (2, 2, 4, 4, 4, 8))
    y_send[(0, 1)] = head + first + bulk(0, len(whole), [("u", u2, u3 - u2)])
    fwd[(0, 0)] = range(len(head), len(head) + len(first))
    for x in range(2):
        first = _split("t", x * _FWD_A, (x + 1) * _FWD_A, (4,))
        y_send[(x, 0)] = first + bulk(2 * _FWD_A, _TILES)
        fwd[(x, 1)] = range(len(first))

    early = {(1, 1): list(range(_HEAD_11, u1 // 2)),
             (0, 1): list(range(u3 // 2, u4 // 2)), (0, 0): [], (1, 0): []}
    cut_row = 8 * (whole[7] + 1)
    row_loads = {0: ((0, _ROWS),), 1: ((0, cut_row), (cut_row, _ROWS - cut_row))}
    return whole, halves, y_send, fwd, early, row_loads


_WHOLE, _HALVES, _Y_SEND, _FWD, _EARLY, _ROW_LOADS = _schedule()


def _tile_rows(t, n=1):
    return pl.ds(8 * t, 8 * n)


def _unit_rows(u):
    t, parity = _HALVES[u // 2]
    return pl.ds(8 * t + 4 * (u % 2) + parity, 2, stride=2)


def _body(x_tiles, x_units, out, x_vmem, stage, send_t, recv_t, send_u, recv_u,
          recv_f, load_sems, y_send_sems, y_recv_sems, x_send_sems, x_recv_sems,
          ready):
    my_x = lax.axis_index("x")
    my_y = lax.axis_index("y")
    barrier = pltpu.get_barrier_semaphore()

    def signal(sem, dev):
        pl.semaphore_signal(sem, inc=1, device_id=dev, device_id_type=_MESH)

    @pl.when(my_x == 1)
    def _():
        signal(barrier, (1, 1 - my_y))

    def program(me):
        y_peer = (me[0], 1 - me[1])
        x_peer = (1 - me[0], me[1])
        diag = (1 - me[0], 1 - me[1])
        holds_b = me[1] == 1
        y_out, y_in = _Y_SEND[me], _Y_SEND[y_peer]
        x_in = [_Y_SEND[diag][i] for i in _FWD[x_peer]]
        early, row_loads = _EARLY[me], _ROW_LOADS[me[1]]

        def hbm_units(u, n):
            t, parity = _HALVES[u // 2]
            return x_units.at[t, pl.ds(u % 2, n), :, parity, 0, :]

        def recv_view(p):
            kind, lo, n = p
            if kind == "t":
                return recv_t.at[_tile_rows(lo, n)]
            return (recv_u if kind == "u" else recv_f).at[pl.ds(lo, n)]

        def send_view(p):
            kind, lo, n = p
            if kind == "t":
                return send_t.at[_tile_rows(lo, n)]
            return send_u.at[pl.ds(lo, n)] if kind == "u" else hbm_units(lo, n)

        def remote(src, p, send_sem, recv_sem, peer):
            return pltpu.make_async_remote_copy(
                src_ref=src, dst_ref=recv_view(p), send_sem=send_sem,
                recv_sem=recv_sem, device_id=peer, device_id_type=_MESH)

        loads = [pltpu.make_async_copy(hbm_units(2 * h, 2),
                                       stage.at[pl.ds(2 * i, 2)], load_sems.at[i])
                 for i, h in enumerate(early)]
        loads += [pltpu.make_async_copy(x_tiles.at[pl.ds(r0, rows)],
                                        x_vmem.at[pl.ds(r0, rows)],
                                        load_sems.at[len(early) + i])
                  for i, (r0, rows) in enumerate(row_loads)]
        pending = set(range(len(loads)))

        def wait_load(i):
            if i in pending:
                loads[i].wait()
                pending.discard(i)

        def wait_tile(t):
            for i, (r0, rows) in enumerate(row_loads):
                if r0 <= 8 * t < r0 + rows:
                    wait_load(len(early) + i)

        converted = set()

        def convert(p):
            kind, lo, n = p
            if kind == "u":
                for h in range(lo // 2, (lo + n + 1) // 2):
                    if h in converted:
                        continue
                    converted.add(h)
                    for u in (2 * h, 2 * h + 1):
                        if h in early:
                            wait_load(early.index(h))
                            v = stage[2 * early.index(h) + u % 2]
                        else:
                            wait_tile(_HALVES[h][0])
                            v = x_vmem[_unit_rows(u), :]
                        send_u[u] = v.astype(jnp.bfloat16)
            elif not holds_b:
                wait_tile(0)
                rows = _tile_rows(lo, n)
                send_t[rows, :] = x_vmem[rows, :].astype(jnp.bfloat16)
            else:
                for s in range(lo, lo + n, 2):
                    for t in _WHOLE[s:s + 2]:
                        wait_tile(t)
                    v = jnp.concatenate(
                        [x_vmem[_tile_rows(t), :] for t in _WHOLE[s:s + 2]], axis=0)
                    send_t[_tile_rows(s, 2), :] = v.astype(jnp.bfloat16)

        def add(p):
            kind, lo, n = p
            if kind != "t":
                buf = recv_u if kind == "u" else recv_f
                for u in range(lo, lo + n):
                    rows = _unit_rows(u)
                    out[rows, :] = x_vmem[rows, :] + buf[u].astype(jnp.float32)
            elif holds_b:
                rows = _tile_rows(lo, n)
                out[rows, :] = x_vmem[rows, :] + recv_t[rows, :].astype(jnp.float32)
            else:
                for s in range(lo, lo + n, 2):
                    v = recv_t[_tile_rows(s, 2), :].astype(jnp.float32)
                    for j, t in enumerate(_WHOLE[s:s + 2]):
                        rows = _tile_rows(t)
                        out[rows, :] = x_vmem[rows, :] + v[8 * j:8 * j + 8]

        y_sends = [remote(send_view(p), p, y_send_sems.at[i], y_recv_sems.at[i],
                          y_peer)
                   for i, p in enumerate(y_out)]

        if holds_b:
            n_head = sum(p[0] == "f" for p in y_out)
            n_first = _LOADS_BEFORE_BARRIER[me]
            for c in loads[:n_first]:
                c.start()
            pl.semaphore_wait(barrier, 1)
            y_sends[0].start()
            loads[n_first].start()
            for c in y_sends[1:n_head]:
                c.start()
            if me == (0, 1):
                signal(barrier, y_peer)
            for c in loads[n_first + 1:]:
                c.start()
            for p, c in list(zip(y_out, y_sends))[n_head:]:
                convert(p)
                c.start()
            for i in sorted(pending):
                wait_load(i)
            pl.semaphore_wait(ready, 1)
        else:
            signal(barrier, (0, 1) if me == (0, 0) else (0, 0))
            for c in loads:
                c.start()
            for p in y_out:
                convert(p)
            pl.semaphore_wait(barrier, 2)
            if me == (0, 0):
                signal(barrier, x_peer)
            for c in y_sends:
                c.start()
            if me == (1, 0):
                signal(ready, diag)
                signal(ready, y_peer)

        y_recvs = [remote(recv_view(p), p, y_send_sems.at[i], y_recv_sems.at[i],
                          y_peer)
                   for i, p in enumerate(y_in)]
        x_recvs = [remote(recv_view(p), p, x_send_sems.at[j], x_recv_sems.at[j],
                          x_peer)
                   for j, p in enumerate(x_in)]
        x_sends = {i: remote(recv_view(y_in[i]), y_in[i], x_send_sems.at[j],
                             x_recv_sems.at[j], x_peer)
                   for j, i in enumerate(_FWD[me])}

        n, m = len(y_in), len(x_in)
        y_late, x_split = (2, m - 6) if me == (0, 0) else (1, m - 1)
        deferred = []
        for i, p in enumerate(y_in[:n - y_late]):
            y_recvs[i].wait_recv()
            deferred.append(p)
            if i in x_sends:
                x_sends[i].start()
            if i not in x_sends or i + 1 not in x_sends:
                for q in deferred:
                    add(q)
                deferred = []
        for c in y_sends + list(x_sends.values()):
            c.wait_send()
        tail = [(x_recvs[j], x_in[j]) for j in range(x_split)]
        tail += [(y_recvs[i], y_in[i]) for i in range(n - y_late, n - 1)]
        tail += [(x_recvs[j], x_in[j]) for j in range(x_split, m - 1)]
        for c, p in tail:
            c.wait_recv()
            add(p)
        y_recvs[-1].wait_recv()
        x_recvs[-1].wait_recv()
        add(y_in[-1])
        add(x_in[-1])

    for d in _DEVICES:
        pl.when(jnp.logical_and(my_x == d[0], my_y == d[1]))(
            functools.partial(program, d))


def _compiler_params():
    try:
        return pltpu.CompilerParams(collective_id=0, disable_bounds_checks=True,
                                    disable_semaphore_checks=True)
    except TypeError:
        return pltpu.CompilerParams(collective_id=0)


def pallas_dist_ar_xy_y_m256_n256_kernel(x: jax.Array):
    assert x.shape == (M, N), x.shape
    n_early = max(len(v) for v in _EARLY.values())
    n_load = max(len(_EARLY[d]) + len(_ROW_LOADS[d[1]]) for d in _DEVICES)
    n_y = max(len(v) for v in _Y_SEND.values())
    n_x = max(len(v) for v in _FWD.values())
    n_units = 2 * len(_HALVES)
    tiles = x.reshape(M // 8, 8, N // 128, 128).transpose(0, 2, 1, 3)
    out = pl.pallas_call(
        _body,
        out_shape=jax.ShapeDtypeStruct((_ROWS, 128), jnp.float32),
        in_specs=[pl.BlockSpec(memory_space=pl.ANY)] * 2,
        out_specs=pl.BlockSpec(memory_space=pltpu.VMEM),
        scratch_shapes=[
            pltpu.VMEM((_ROWS, 128), jnp.float32),
            pltpu.VMEM((2 * n_early, 2, 128), jnp.float32),
            pltpu.VMEM((_ROWS, 128), jnp.bfloat16),
            pltpu.VMEM((_ROWS, 128), jnp.bfloat16),
            pltpu.VMEM((n_units, 2, 128), jnp.bfloat16),
            pltpu.VMEM((n_units, 2, 128), jnp.bfloat16),
            pltpu.VMEM((n_units, 2, 128), jnp.float32),
            pltpu.SemaphoreType.DMA((n_load,)),
            pltpu.SemaphoreType.DMA((n_y,)),
            pltpu.SemaphoreType.DMA((n_y,)),
            pltpu.SemaphoreType.DMA((n_x,)),
            pltpu.SemaphoreType.DMA((n_x,)),
            pltpu.SemaphoreType.REGULAR,
        ],
        compiler_params=_compiler_params(),
    )(tiles.reshape(_ROWS, 128), tiles.reshape(_TILES, 2, 2, 2, 1, 128))
    return out.reshape(M // 8, N // 128, 8, 128).transpose(0, 2, 1, 3).reshape(M, N)
```
